```python
import numpy as np

kernel_name = "dist_mean_ax0_shard0_i_m4096_n1024"

def setup_inputs():
    return {"x": np.random.randn(16384, 1024).astype(np.float32)}

def reference(x: np.ndarray) -> np.ndarray:
    return np.mean(x, axis=0, keepdims=True)
```

```python
import jax
import jax.numpy as jnp
from jax import lax
from jax.experimental import pallas as pl
from jax.experimental.pallas import tpu as pltpu

N_DEV = 4
TILES = 8
GROUP = 16
LOOKAHEAD = 4
TAIL = (8, 4, 2, 2)
PACE_NS = 31
HEAD_PACE_NS = 35


def _chunk(step, r):
    lane = ((r & 1) << 8) | ((r >> 1) & 1) | (((r >> 2) & 1) << 5) | (((r >> 3) & 1) << 4)
    return lane + (((step & 7) << 1) | ((step >> 3) << 6))


def pallas_dist_mean_ax0_shard0_i_m4096_n1024_kernel(
    x: jax.Array,
):
    m, n = x.shape
    assert (m, n) == (4096, 1024)
    n_tiles = m * n // (8 * 128)
    n_chunks = n_tiles // TILES
    steps = n_chunks // GROUP
    scale = 1.0 / (N_DEV * m)

    def body(x_hbm, o_ref, buf, comm, load_sems, tail_sems, send_sems, recv_sems):
        tail_of = [t for t, size in enumerate(TAIL) for _ in range(size)]

        def sem(step, r):
            if isinstance(step, int):
                if step == steps - 1:
                    return tail_sems.at[tail_of[r]]
                return load_sems.at[step % (LOOKAHEAD + 1)]
            return load_sems.at[lax.rem(step, LOOKAHEAD + 1)]

        def issue(step, r):
            c = _chunk(step, r)
            dst = buf.at[step, r]
            if isinstance(c, int) and c == n_chunks - 1:
                pieces = [
                    (x_hbm.at[pl.ds(0, TILES - 1)], dst.at[pl.ds(1, TILES - 1)]),
                    (x_hbm.at[pl.ds(n_tiles - 1, 1)], dst.at[pl.ds(0, 1)]),
                ]
            else:
                pieces = [(x_hbm.at[pl.ds(TILES - 1 + TILES * c, TILES)], dst)]
            for src, dst in pieces:
                pltpu.make_async_copy(src, dst, sem(step, r)).start(priority=r % 2)

        def wait(ref, s):
            pltpu.make_async_copy(ref, ref, s).wait()

        def add(acc, step, r):
            return [acc[k] + buf[step, r, k] for k in range(TILES)]

        for step in range(LOOKAHEAD):
            for r in range(GROUP):
                issue(step, r)
                if step * GROUP + r >= 2:
                    pl.delay(HEAD_PACE_NS)

        me = lax.axis_index("i")
        peers = [(me + d) & (N_DEV - 1) for d in range(N_DEV)]
        barrier = pltpu.get_barrier_semaphore()
        for d in range(1, N_DEV):
            pl.semaphore_signal(
                barrier, inc=1, device_id=(peers[d],),
                device_id_type=pl.DeviceIdType.MESH,
            )

        def steady(step, acc):
            wait(buf.at[step], sem(step, 0))
            for r in range(GROUP):
                issue(step + LOOKAHEAD, r)
                acc = add(acc, step, r)
                pl.delay(PACE_NS)
            return acc

        acc = [jnp.zeros((8, 128), jnp.float32)] * TILES
        acc = lax.fori_loop(0, steps - LOOKAHEAD - 1, steady, acc)
        acc = steady(steps - LOOKAHEAD - 1, acc)

        pl.semaphore_wait(barrier, N_DEV - 1)
        for step in range(steps - LOOKAHEAD, steps - 1):
            wait(buf.at[step], sem(step, 0))
            for r in range(GROUP):
                acc = add(acc, step, r)
        r0 = 0
        for t, size in enumerate(TAIL):
            wait(buf.at[steps - 1, pl.ds(r0, size)], tail_sems.at[t])
            for r in range(r0, r0 + size):
                acc = add(acc, steps - 1, r)
            r0 += size

        comm[0] = jnp.concatenate(
            [jnp.sum(a, axis=0, keepdims=True) * scale for a in acc], axis=0
        )

        def rdma(d):
            return pltpu.make_async_remote_copy(
                comm.at[0], comm.at[d], send_sems.at[d - 1], recv_sems.at[d - 1],
                device_id=(peers[d],), device_id_type=pl.DeviceIdType.MESH,
            )

        rdma(2).start()
        rdma(2).wait_send()
        for d in (1, 3):
            rdma(d).start()
        for d in (1, 3):
            rdma(d).wait_send()
        total = comm[0]
        for d in (1, 3, 2):
            rdma(d).wait_recv()
            total = total + comm[d]
        o_ref[...] = pltpu.roll(total, TILES - 1, 0)

    tiles = (
        x.reshape(m // 8, 8, n // 128, 128)
        .transpose(0, 2, 1, 3)
        .reshape(n_tiles, 8, 128)
    )
    out = pl.pallas_call(
        body,
        out_shape=jax.ShapeDtypeStruct((n // 128, 128), jnp.float32),
        in_specs=[pl.BlockSpec(memory_space=pl.ANY)],
        out_specs=pl.BlockSpec(memory_space=pltpu.VMEM),
        scratch_shapes=[
            pltpu.VMEM((steps, GROUP, TILES, 8, 128), jnp.float32),
            pltpu.VMEM((N_DEV, n // 128, 128), jnp.float32),
            pltpu.SemaphoreType.DMA((LOOKAHEAD + 1,)),
            pltpu.SemaphoreType.DMA((len(TAIL),)),
            pltpu.SemaphoreType.DMA((N_DEV - 1,)),
            pltpu.SemaphoreType.DMA((N_DEV - 1,)),
        ],
        compiler_params=pltpu.CompilerParams(
            collective_id=0,
            vmem_limit_bytes=48 * 1024 * 1024,
            disable_semaphore_checks=True,
            disable_bounds_checks=True,
        ),
    )(tiles)
    return out.reshape(1, n)
```

```python
import jax
import jax.numpy as jnp
from jax import lax
from jax.experimental import pallas as pl
from jax.experimental.pallas import tpu as pltpu

N_DEV = 4
ROWS, COLS = 4096, 1024
BLOCKS = COLS // 128
N_TILES = ROWS * COLS // (8 * 128)
N_CHUNKS = N_TILES // BLOCKS

ORDER_BITS = (256, 1, 32, 16, 128, 64, 4, 8, 2)
HEAD_START = 28
GATE_LEAD = 10
GROUP = 16
SUM_LAG = 96
LAST_GROUPS = (4, 2)
LATE_BITS, LATE_BASE = (64, 1, 16, 8, 32), 384
LATE_GROUPS = (16, 8, 8)


def _span(bits, base=0):
    out = [base]
    for bit in bits:
        out += [c ^ bit for c in out]
    return out


def _chunk_copies(chunk, late):
    if chunk == N_CHUNKS - 1:
        return [(N_TILES - 1, 1), (0, BLOCKS - 1)]
    first = BLOCKS - 1 + BLOCKS * chunk
    if chunk in late:
        return [(first + 1, BLOCKS - 1)]
    return [(first, BLOCKS)]


def _schedule():
    order = _span(ORDER_BITS)
    fast, slow = order[0::2], order[1::2]
    paired = len(fast) - HEAD_START
    stream = [(c, 1) for c in slow[:HEAD_START]]
    for k in range(paired):
        stream += [(fast[k], 0), (slow[k + HEAD_START], 1)]
    gated = fast[paired:]
    first_gate = paired - GATE_LEAD
    gates = slow[first_gate : first_gate + HEAD_START]
    after_gates = slow[first_gate + HEAD_START :]

    tail = gated + gates + after_gates
    steady = [c for c, _ in stream if c not in tail]
    steady_groups = [steady[i : i + GROUP] for i in range(0, len(steady), GROUP)]

    drain = gated[: HEAD_START - GATE_LEAD]
    for pair in zip(gated[HEAD_START - GATE_LEAD :], after_gates):
        drain += pair
    drain_groups = []
    for size in reversed(LAST_GROUPS):
        drain_groups.insert(0, drain[-size:])
        drain = drain[:-size]
    while drain:
        drain_groups.insert(0, drain[-8:])
        drain = drain[:-8]
    return stream, gated, steady_groups, [[c] for c in gates], drain_groups


def _tree_sum(values):
    while len(values) > 1:
        pairs = [a + b for a, b in zip(values[0::2], values[1::2])]
        values = pairs + values[2 * len(pairs) :]
    return values[0]


def pallas_dist_mean_ax0_shard0_i_m4096_n1024_kernel(
    x: jax.Array,
):
    assert x.shape == (ROWS, COLS) and x.dtype == jnp.float32
    scale = 1.0 / (N_DEV * ROWS)

    late = _span(LATE_BITS, LATE_BASE)
    stream, gated, steady_groups, gate_groups, drain_groups = _schedule()
    groups = steady_groups + gate_groups + drain_groups
    issued_at = {c: i for i, (c, _) in enumerate(stream)}
    group_of, slot_of, regions, used = {}, {}, [], 0
    for g, group in enumerate(groups):
        start = used
        for c in group:
            group_of[c], slot_of[c] = g, used
            used += sum(tiles for _, tiles in _chunk_copies(c, late))
        regions.append(pl.ds(start, used - start))
    assert sorted(group_of) == list(range(N_CHUNKS))
    assert used + len(late) == N_TILES and sum(LATE_GROUPS) == len(late)
    late_group_of = [g for g, size in enumerate(LATE_GROUPS) for _ in range(size)]

    def body(
        x_hbm, o_ref,
        buf, late_buf,
        tx_early, tx_late, tx_all, rx_early, rx_late, rx_all,
        load_sems, late_sems, send_sems, recv_sems,
    ):
        acc = [None] * BLOCKS

        def fetch(chunk, priority):
            slot = slot_of[chunk]
            for first, tiles in _chunk_copies(chunk, late):
                pltpu.make_async_copy(
                    x_hbm.at[pl.ds(first, tiles)],
                    buf.at[pl.ds(slot, tiles)],
                    load_sems.at[group_of[chunk]],
                ).start(priority=priority)
                slot += tiles

        def fetch_late(k):
            pltpu.make_async_copy(
                x_hbm.at[BLOCKS - 1 + BLOCKS * late[k]],
                late_buf.at[k],
                late_sems.at[late_group_of[k]],
            ).start(priority=1)

        def wait_filled(ref, sem):
            pltpu.make_async_copy(ref, ref, sem).wait()

        def wait_group(g):
            wait_filled(buf.at[regions[g]], load_sems.at[g])

        def add_group(g):
            for chunk in groups[g]:
                slot = slot_of[chunk]
                for first, tiles in _chunk_copies(chunk, late):
                    for tile in range(first, first + tiles):
                        b = tile % BLOCKS
                        acc[b] = buf[slot] if acc[b] is None else acc[b] + buf[slot]
                        slot += 1

        summed = 0
        for i, (chunk, priority) in enumerate(stream):
            fetch(chunk, priority)
            if i == HEAD_START + 8:
                me = lax.axis_index("i")
                peers = [(me + d) & (N_DEV - 1) for d in range(N_DEV)]
                barrier = pltpu.get_barrier_semaphore()
                for peer in peers[1:]:
                    pl.semaphore_signal(
                        barrier, inc=1, device_id=(peer,),
                        device_id_type=pl.DeviceIdType.MESH,
                    )
            if issued_at[steady_groups[summed][-1]] + SUM_LAG <= i:
                wait_group(summed)
                add_group(summed)
                summed += 1
        pl.semaphore_wait(barrier, N_DEV - 1)

        fetched_late = 0
        for k, chunk in enumerate(gated):
            gate = len(steady_groups) + k
            wait_group(gate)
            fetch(chunk, 0)
            while len(late) - fetched_late > len(gated) - 1 - k:
                fetch_late(fetched_late)
                fetched_late += 1
            add_group(gate)
            if summed < len(steady_groups):
                wait_group(summed)
                add_group(summed)
                summed += 1
        assert summed == len(steady_groups) and fetched_late == len(late)
        for g in range(len(steady_groups) + len(gate_groups), len(groups)):
            wait_group(g)
            add_group(g)

        def column_mean(v):
            return jnp.sum(v, axis=0, keepdims=True) * scale

        def send(k, src, dst, d):
            return pltpu.make_async_remote_copy(
                src, dst, send_sems.at[k], recv_sems.at[k],
                device_id=(peers[d],), device_id_type=pl.DeviceIdType.MESH,
            )

        to_diagonal_early = send(0, tx_early, rx_early, 2)
        to_diagonal_late = send(1, tx_late, rx_late, 2)
        to_neighbors = [send(2, tx_all, rx_all.at[0], 1), send(3, tx_all, rx_all.at[1], 3)]

        early = jnp.concatenate([column_mean(v) for v in acc[:-1]], axis=0)
        tx_early[...] = early
        to_diagonal_early.start()

        k = 0
        for g, size in enumerate(LATE_GROUPS):
            wait_filled(late_buf.at[pl.ds(k, size)], late_sems.at[g])
            acc[-1] = _tree_sum([late_buf[j] for j in range(k, k + size)] + [acc[-1]])
            k += size
        last = column_mean(acc[-1])
        tx_late[...] = last
        to_diagonal_late.start()

        tx_all[pl.ds(0, BLOCKS - 1)] = early
        tx_all[pl.ds(BLOCKS - 1, 1)] = last
        to_diagonal_late.wait_send()
        for copy in to_neighbors:
            copy.start()
        to_diagonal_early.wait_send()
        for copy in to_neighbors:
            copy.wait_send()

        for copy in to_neighbors:
            copy.wait_recv()
        total = tx_all[...] + rx_all[0] + rx_all[1]
        to_diagonal_early.wait_recv()
        o_ref[pl.ds(0, BLOCKS - 1)] = total[: BLOCKS - 1] + rx_early[...]
        to_diagonal_late.wait_recv()
        o_ref[pl.ds(BLOCKS - 1, 1)] = total[BLOCKS - 1 :] + rx_late[...]

    tiles = (
        x.reshape(ROWS // 8, 8, BLOCKS, 128)
        .transpose(0, 2, 1, 3)
        .reshape(N_TILES, 8, 128)
    )
    f32 = jnp.float32
    out = pl.pallas_call(
        body,
        out_shape=jax.ShapeDtypeStruct((BLOCKS, 128), f32),
        in_specs=[pl.BlockSpec(memory_space=pl.ANY)],
        out_specs=pl.BlockSpec(memory_space=pltpu.VMEM),
        scratch_shapes=[
            pltpu.VMEM((used, 8, 128), f32),
            pltpu.VMEM((len(late), 8, 128), f32),
            pltpu.VMEM((BLOCKS - 1, 128), f32),
            pltpu.VMEM((1, 128), f32),
            pltpu.VMEM((BLOCKS, 128), f32),
            pltpu.VMEM((BLOCKS - 1, 128), f32),
            pltpu.VMEM((1, 128), f32),
            pltpu.VMEM((2, BLOCKS, 128), f32),
            pltpu.SemaphoreType.DMA((len(groups),)),
            pltpu.SemaphoreType.DMA((len(LATE_GROUPS),)),
            pltpu.SemaphoreType.DMA((4,)),
            pltpu.SemaphoreType.DMA((4,)),
        ],
        compiler_params=pltpu.CompilerParams(
            collective_id=0,
            vmem_limit_bytes=32 * 1024 * 1024,
            disable_bounds_checks=True,
            disable_semaphore_checks=True,
        ),
    )(tiles)
    return out.reshape(1, COLS)
```

```python
import jax
import jax.numpy as jnp
from jax import lax
from jax.experimental import pallas as pl
from jax.experimental.pallas import tpu as pltpu

N_DEV = 4
ROWS, COLS = 4096, 1024
BLOCKS = COLS // 128
N_TILES = ROWS * COLS // (8 * 128)
N_CHUNKS = N_TILES // BLOCKS

ORDER_BITS = (256, 1, 32, 16, 128, 64, 4, 8, 2)
HEAD_START = 28
GATE_LEAD = 10
GROUP = 16
SUM_LAG = 96
LAST_GROUPS = (4, 2)
LATE_BITS, LATE_BASE = (64, 1, 16, 8, 32), 384
LATE_GROUPS = (16, 8, 8)


def _span(bits, base=0):
    out = [base]
    for bit in bits:
        out += [c ^ bit for c in out]
    return out


def _chunk_copies(chunk, late):
    if chunk == N_CHUNKS - 1:
        return [(N_TILES - 1, 1), (0, BLOCKS - 1)]
    first = BLOCKS - 1 + BLOCKS * chunk
    if chunk in late:
        return [(first + 1, BLOCKS - 1)]
    return [(first, BLOCKS)]


def _schedule():
    order = _span(ORDER_BITS)
    fast, slow = order[0::2], order[1::2]
    paired = len(fast) - HEAD_START
    stream = [(c, 1) for c in slow[:HEAD_START]]
    for k in range(paired):
        stream += [(fast[k], 0), (slow[k + HEAD_START], 1)]
    gated = fast[paired:]
    first_gate = paired - GATE_LEAD
    gates = slow[first_gate : first_gate + HEAD_START]
    after_gates = slow[first_gate + HEAD_START :]

    tail = gated + gates + after_gates
    steady = [c for c, _ in stream if c not in tail]
    steady_groups = [steady[i : i + GROUP] for i in range(0, len(steady), GROUP)]

    drain = gated[: HEAD_START - GATE_LEAD]
    for pair in zip(gated[HEAD_START - GATE_LEAD :], after_gates):
        drain += pair
    drain_groups = []
    for size in reversed(LAST_GROUPS):
        drain_groups.insert(0, drain[-size:])
        drain = drain[:-size]
    while drain:
        drain_groups.insert(0, drain[-8:])
        drain = drain[:-8]
    return stream, gated, steady_groups, [[c] for c in gates], drain_groups


def _tree_sum(values):
    while len(values) > 1:
        pairs = [a + b for a, b in zip(values[0::2], values[1::2])]
        values = pairs + values[2 * len(pairs) :]
    return values[0]


def pallas_dist_mean_ax0_shard0_i_m4096_n1024_kernel(
    x: jax.Array,
):
    assert x.shape == (ROWS, COLS) and x.dtype == jnp.float32
    f32 = jnp.float32
    scale = 1.0 / (N_DEV * ROWS)

    late = _span(LATE_BITS, LATE_BASE)
    stream, gated, steady_groups, gate_groups, drain_groups = _schedule()
    groups = steady_groups + gate_groups + drain_groups
    issued_at = {c: i for i, (c, _) in enumerate(stream)}
    group_of, slot_of, layout, used = {}, {}, [], 0
    for g, group in enumerate(groups):
        whole = [c for c in group if c not in late]
        short = [c for c in group if c in late]
        layout.append((used, len(whole), len(short)))
        for c in whole + short:
            group_of[c], slot_of[c] = g, used
            used += BLOCKS - (c in late)
    assert sorted(group_of) == list(range(N_CHUNKS))
    assert used + len(late) == N_TILES and sum(LATE_GROUPS) == len(late)
    late_group_of = [g for g, size in enumerate(LATE_GROUPS) for _ in range(size)]

    def body(
        x_hbm, o_ref,
        buf, late_buf,
        tx_early, tx_late, tx_all, rx_early, rx_late, rx_all,
        load_sems, late_sems, send_sems, recv_sems,
    ):
        def fetch(chunk, priority):
            slot = slot_of[chunk]
            for first, tiles in _chunk_copies(chunk, late):
                pltpu.make_async_copy(
                    x_hbm.at[pl.ds(first, tiles)],
                    buf.at[pl.ds(slot, tiles)],
                    load_sems.at[group_of[chunk]],
                ).start(priority=priority)
                slot += tiles

        def fetch_late(k):
            pltpu.make_async_copy(
                x_hbm.at[BLOCKS - 1 + BLOCKS * late[k]],
                late_buf.at[k],
                late_sems.at[late_group_of[k]],
            ).start(priority=1)

        def wait_filled(ref, sem):
            pltpu.make_async_copy(ref, ref, sem).wait()

        def wait_group(g):
            start, whole, short = layout[g]
            tiles = whole * BLOCKS + short * (BLOCKS - 1)
            wait_filled(buf.at[pl.ds(start, tiles)], load_sems.at[g])

        def chunk_sum(start, chunks, tiles):
            part = buf[pl.ds(start, chunks * tiles)]
            return jnp.sum(part.reshape(chunks, tiles, 8, 128), axis=0)

        acc = [jnp.zeros((1, 8, 128), f32), jnp.zeros((BLOCKS - 1, 8, 128), f32)]

        def add_group(g):
            start, whole, short = layout[g]
            if whole:
                part = chunk_sum(start, whole, BLOCKS)
                acc[0] += part[:1]
                acc[1] += part[1:]
            if short:
                acc[1] += chunk_sum(start + whole * BLOCKS, short, BLOCKS - 1)

        summed = 0
        for i, (chunk, priority) in enumerate(stream):
            fetch(chunk, priority)
            if i == HEAD_START + 8:
                me = lax.axis_index("i")
                peers = [(me + d) & (N_DEV - 1) for d in range(N_DEV)]
                barrier = pltpu.get_barrier_semaphore()
                for peer in peers[1:]:
                    pl.semaphore_signal(
                        barrier, inc=1, device_id=(peer,),
                        device_id_type=pl.DeviceIdType.MESH,
                    )
            if issued_at[steady_groups[summed][-1]] + SUM_LAG <= i:
                wait_group(summed)
                add_group(summed)
                summed += 1
        pl.semaphore_wait(barrier, N_DEV - 1)

        fetched_late = 0
        for k, chunk in enumerate(gated):
            gate = len(steady_groups) + k
            wait_group(gate)
            fetch(chunk, 0)
            while len(late) - fetched_late > len(gated) - 1 - k:
                fetch_late(fetched_late)
                fetched_late += 1
            add_group(gate)
            if summed < len(steady_groups):
                wait_group(summed)
                add_group(summed)
                summed += 1
        assert summed == len(steady_groups) and fetched_late == len(late)
        for g in range(len(steady_groups) + len(gate_groups), len(groups)):
            wait_group(g)
            add_group(g)

        def column_mean(v):
            return jnp.sum(v, axis=1) * scale

        def send(k, src, dst, d):
            return pltpu.make_async_remote_copy(
                src, dst, send_sems.at[k], recv_sems.at[k],
                device_id=(peers[d],), device_id_type=pl.DeviceIdType.MESH,
            )

        to_diagonal_early = send(0, tx_early, rx_early, 2)
        to_diagonal_late = send(1, tx_late, rx_late, 2)
        to_neighbors = [
            send(2, tx_all, rx_all.at[0], 1),
            send(3, tx_all, rx_all.at[1], 3),
        ]

        early = column_mean(acc[1])
        tx_early[...] = early
        to_diagonal_early.start()

        k = 0
        for g, size in enumerate(LATE_GROUPS):
            wait_filled(late_buf.at[pl.ds(k, size)], late_sems.at[g])
            acc[0] = _tree_sum([late_buf[pl.ds(j, 1)] for j in range(k, k + size)] + [acc[0]])
            k += size
        last = column_mean(acc[0])
        tx_late[...] = last
        to_diagonal_late.start()

        tx_all[pl.ds(0, BLOCKS - 1)] = early
        tx_all[pl.ds(BLOCKS - 1, 1)] = last
        to_diagonal_late.wait_send()
        for copy in to_neighbors:
            copy.start()
        to_diagonal_early.wait_send()
        for copy in to_neighbors:
            copy.wait_send()

        for copy in to_neighbors:
            copy.wait_recv()
        total = tx_all[...] + rx_all[0] + rx_all[1]
        to_diagonal_early.wait_recv()
        o_ref[pl.ds(0, BLOCKS - 1)] = total[: BLOCKS - 1] + rx_early[...]
        to_diagonal_late.wait_recv()
        o_ref[pl.ds(BLOCKS - 1, 1)] = total[BLOCKS - 1 :] + rx_late[...]

    tiles = (
        x.reshape(ROWS // 8, 8, BLOCKS, 128)
        .transpose(0, 2, 1, 3)
        .reshape(N_TILES, 8, 128)
    )
    out = pl.pallas_call(
        body,
        out_shape=jax.ShapeDtypeStruct((BLOCKS, 128), f32),
        in_specs=[pl.BlockSpec(memory_space=pl.ANY)],
        out_specs=pl.BlockSpec(memory_space=pltpu.VMEM),
        scratch_shapes=[
            pltpu.VMEM((used, 8, 128), f32),
            pltpu.VMEM((len(late), 8, 128), f32),
            pltpu.VMEM((BLOCKS - 1, 128), f32),
            pltpu.VMEM((1, 128), f32),
            pltpu.VMEM((BLOCKS, 128), f32),
            pltpu.VMEM((BLOCKS - 1, 128), f32),
            pltpu.VMEM((1, 128), f32),
            pltpu.VMEM((2, BLOCKS, 128), f32),
            pltpu.SemaphoreType.DMA((len(groups),)),
            pltpu.SemaphoreType.DMA((len(LATE_GROUPS),)),
            pltpu.SemaphoreType.DMA((4,)),
            pltpu.SemaphoreType.DMA((4,)),
        ],
        compiler_params=pltpu.CompilerParams(
            collective_id=0,
            vmem_limit_bytes=32 * 1024 * 1024,
            disable_semaphore_checks=True,
        ),
    )(tiles)
    return out.reshape(1, COLS)
```
